```python
import numpy as np

kernel_name = "dist_mlp2_tp_i_m512_h1024_out512"

def setup_inputs():
    x = np.random.randn(512, 512).astype(np.float32)
    W1 = np.random.randn(512, 4096).astype(np.float32)
    W2 = np.random.randn(4096, 512).astype(np.float32)
    return {"x": x, "W1": W1, "W2": W2}

def reference(x: np.ndarray, W1: np.ndarray, W2: np.ndarray) -> np.ndarray:
    h = x @ W1
    h = np.maximum(h, 0.0)
    return h @ W2
```

```python
import contextlib

import jax
import jax.numpy as jnp
from jax import lax
from jax.experimental import pallas as pl
from jax.experimental.pallas import tpu as pltpu

BF = jnp.bfloat16
F32 = jnp.float32
MESH = pl.DeviceIdType.MESH


def scope(n):
    return contextlib.nullcontext()


def pallas_dist_mlp2_tp_i_m512_h1024_out512_kernel(x, W1, W2):
    M, K = x.shape
    H = W1.shape[1]
    N = W2.shape[1]
    RB = M // 4
    NQ = 4
    QC = N // NQ
    NK = 4
    KC = K // NK

    def body(x_hbm, w1_hbm, w2_hbm, out_ref,
             xs_f, xs_b, xk_b, w1_f, w1_b, w2_f, w2_b, acc, hs, hk,
             s1, r1, s2, r2, s3, r3, lsem, xs_sem, xr_sem, ssem, rsem):
        me = lax.axis_index("i")
        cx = me // 2
        cy = (me ^ (me // 2)) % 2
        px = 3 - me
        py = me ^ 1
        send_row = [pl.multiple_of((1 - cx) * RB, RB), pl.multiple_of(2 * RB + (1 - cy) * RB, RB)]
        keep_row = [pl.multiple_of(cx * RB, RB), pl.multiple_of(2 * RB + cy * RB, RB)]
        p_outer = [px, py]
        p_inner = [py, px]

        ld_x = [pltpu.make_async_copy(x_hbm.at[pl.ds(send_row[t], RB), :], xs_f.at[pl.ds(t * RB, RB), :], lsem.at[t]) for t in range(2)]
        ld_w1 = [pltpu.make_async_copy(w1_hbm.at[pl.ds(k * KC, KC), :], w1_f.at[pl.ds(k * KC, KC), :], lsem.at[2 + k]) for k in range(NK)]
        ld_w2 = [pltpu.make_async_copy(w2_hbm.at[:, pl.ds(q * QC, QC)], w2_f.at[q], lsem.at[2 + NK + q]) for q in range(NQ)]
        for c in ld_x + ld_w1 + ld_w2:
            c.start()

        bar = pltpu.get_barrier_semaphore()
        for p in (px, py):
            pl.semaphore_signal(bar, inc=1, device_id=(p,), device_id_type=MESH)

        def rdma(phase, t, q):
            src = (s1, s2, s3)[phase]
            dst = (r1, r2, r3)[phase]
            dev = p_inner[t] if phase == 1 else p_outer[t]
            idx = (phase * 2 + t) * NQ + q
            return pltpu.make_async_remote_copy(src.at[t, q], dst.at[t, q], ssem.at[idx], rsem.at[idx],
                                                device_id=(dev,), device_id_type=MESH)
        x_rdma = [pltpu.make_async_remote_copy(xs_b.at[pl.ds(t * RB, RB), :], xk_b.at[pl.ds(t * RB, RB), :],
                                               xs_sem.at[t], xr_sem.at[t], device_id=(p_outer[t],), device_id_type=MESH) for t in range(2)]

        with scope("xwait"):
            for t in range(2):
                ld_x[t].wait()
                xs_b[pl.ds(t * RB, RB), :] = xs_f[pl.ds(t * RB, RB), :].astype(BF)
        with scope("barrier"):
            pl.semaphore_wait(bar, 2)
        for t in range(2):
            x_rdma[t].start()

        for k in range(NK):
            with scope(f"w1wait{k}"):
                ld_w1[k].wait()
            with scope(f"h{k}"):
                wb = w1_f[pl.ds(k * KC, KC), :].astype(BF)
                w1_b[pl.ds(k * KC, KC), :] = wb
                d = jnp.dot(xs_b[:, pl.ds(k * KC, KC)], wb, preferred_element_type=F32)
                if k == 0:
                    acc[...] = d
                elif k < NK - 1:
                    acc[...] += d
                else:
                    hs[...] = jnp.maximum(acc[...] + d, 0.0).astype(BF)

        def send_tiles(q):
            with scope(f"w2wait{q}"):
                ld_w2[q].wait()
            with scope(f"os{q}"):
                wb = w2_f[q].astype(BF)
                w2_b[q] = wb
                o = jnp.dot(hs[...], wb, preferred_element_type=F32).astype(BF)
                for t in range(2):
                    s1[t, q] = o[t * RB:(t + 1) * RB]
                for t in range(2):
                    rdma(0, t, q).start()

        def hk_part(t):
            with scope(f"xkwait{t}"):
                x_rdma[t].wait_recv()
            with scope(f"hk{t}"):
                d = jnp.dot(xk_b[pl.ds(t * RB, RB), :], w1_b[...], preferred_element_type=F32)
                hk[pl.ds(t * RB, RB), :] = jnp.maximum(d, 0.0).astype(BF)

        def keep_tiles(q):
            with scope(f"ok{q}"):
                o = jnp.dot(hk[...], w2_b[q], preferred_element_type=F32)
                for t in range(2):
                    out_ref[pl.ds(keep_row[t], RB), pl.ds(q * QC, QC)] = o[t * RB:(t + 1) * RB]

        def p2(q):
            for t in range(2):
                with scope(f"r1wait{t}{q}"):
                    rdma(0, t, q).wait_recv()
                v = out_ref[pl.ds(keep_row[t], RB), pl.ds(q * QC, QC)] + r1[t, q].astype(F32)
                out_ref[pl.ds(keep_row[t], RB), pl.ds(q * QC, QC)] = v
                s2[t, q] = v.astype(BF)
                rdma(1, t, q).start()

        def p3(q):
            for t in range(2):
                with scope(f"r2wait{t}{q}"):
                    rdma(1, t, q).wait_recv()
                v = out_ref[pl.ds(keep_row[t], RB), pl.ds(q * QC, QC)] + r2[t, q].astype(F32)
                out_ref[pl.ds(keep_row[t], RB), pl.ds(q * QC, QC)] = v
                s3[t, q] = v.astype(BF)
                rdma(2, t, q).start()

        def fin(q):
            for t in range(2):
                with scope(f"r3wait{t}{q}"):
                    rdma(2, t, q).wait_recv()
                out_ref[pl.ds(send_row[t], RB), pl.ds(q * QC, QC)] = r3[t, q].astype(F32)

        send_tiles(0)
        send_tiles(1)
        hk_part(0)
        send_tiles(2)
        hk_part(1)
        send_tiles(3)
        for q in range(NQ):
            keep_tiles(q)
            p2(q)
        for q in range(NQ):
            p3(q)
        for q in range(NQ):
            fin(q)
        with scope("sendwait"):
            for t in range(2):
                x_rdma[t].wait_send()
            for ph in range(3):
                for t in range(2):
                    for q in range(NQ):
                        rdma(ph, t, q).wait_send()

    comm = pltpu.VMEM((2, NQ, RB, QC), BF)
    return pl.pallas_call(
        body,
        out_shape=jax.ShapeDtypeStruct((M, N), F32),
        in_specs=[pl.BlockSpec(memory_space=pl.ANY)] * 3,
        out_specs=pl.BlockSpec(memory_space=pltpu.VMEM),
        scratch_shapes=[
            pltpu.VMEM((2 * RB, K), F32), pltpu.VMEM((2 * RB, K), BF), pltpu.VMEM((2 * RB, K), BF),
            pltpu.VMEM((K, H), F32), pltpu.VMEM((K, H), BF),
            pltpu.VMEM((NQ, H, QC), F32), pltpu.VMEM((NQ, H, QC), BF),
            pltpu.VMEM((2 * RB, H), F32), pltpu.VMEM((2 * RB, H), BF), pltpu.VMEM((2 * RB, H), BF),
            comm, comm, comm, comm, comm, comm,
            pltpu.SemaphoreType.DMA((2 + NK + NQ,)),
            pltpu.SemaphoreType.DMA((2,)), pltpu.SemaphoreType.DMA((2,)),
            pltpu.SemaphoreType.DMA((6 * NQ,)), pltpu.SemaphoreType.DMA((6 * NQ,)),
        ],
        compiler_params=pltpu.CompilerParams(collective_id=0, disable_semaphore_checks=True),
    )(x, W1, W2)
```

```python
import functools

import jax
import jax.numpy as jnp
from jax import lax
from jax.experimental import pallas as pl
from jax.experimental.pallas import tpu as pltpu

_BF16 = jnp.bfloat16
_F32 = jnp.float32
_MESH = pl.DeviceIdType.MESH

_M, _K, _H, _N = 512, 512, 1024, 512
_RG = 64
_RB = 128
_KC = 128
_HC = 512
_QC = 128
_NT = 32

_DRAIN_AT = {12: 36, 8: 16, 2: 0}

_POS = (0, 3, 1, 2)
_NBRS = ((1, 2), (0, 3), (3, 0), (2, 1))
_PATHS = {"A0": (1, 0, 2, 3), "A1": (0, 1, 3, 2), "B0": (2, 0, 1, 3), "B1": (0, 2, 3, 1)}

_ROUTE = (
    "A0-", "A0-", "A0-", "A1-",
    "A0-", "A0-", "A1-", "A1-",
    "B0-", "A1f", "A1-", "A1-",
    "A1f", "A1f", "A1-", "A1-",
)
_XLOADS = {0: ((1, 0, 4), (3, 0, 4)), 1: ((0, 1, 3), (3, 1, 3)), 3: ((0, 0, 3), (2, 0, 3))}
_W1ORDER = {0: (1, 2, 3, 0), 1: (1, 2, 3, 0), 3: (0, 1, 2, 3)}

_PROG = {}
_PROG[0] = (
    "x10 x33 x30 x32 x12 x11 x31 x13 s722 s321 s311 h311 h610 s712 s701 h611 h211 s601 s301 s302 s331 "
    "h720 h310 s202 s702 s732 s211 s612 h320 s221 h210 s201 s622 h221 h711 h220 h620 h721 h730 h230 "
    "h331 h621 h330 h731 h321 h710 h630 h300 h231 w13 w53 h601 h131 h701 h631 h200 h201 h130 h301 "
    "h531 h700 / h600 w11 w12 w52 h121 s602 o70 o30 h521 p30 p70 w51 w02 h530 s231 s632 h110 h510 "
    "h120 h021 h511 w03 w42 w43 o31 o71 h520 p71 p31 o21 h420 o61 w50 w41 w10 p21 p61 o22 o62 / o32 "
    "o72 p22 p62 h101 h411 h100 h500 p32 p72 h501 h111 h031 h410 o12 o52 p52 p12 o33 o63 / o23 o73 "
    "p63 p33 o13 o53 p73 a00 w40 p23 a20 w01 w00 o10 p13 p53 o60 h400 h431 h401 h010 h000 o20 h421 "
    "h020 h430 e20 a10 o51 e10 o50 a60 a50 a51 a40 a11 e51 a41 e50 e60 a01 o43 h001 h011 h030 o40 p43 "
    "o03 o00 o11 p03 t50 a42 o42 e00 a02 t10 o41 e40 o01 t60 e41 e11 e01 t40 o02 t00 e42 e02 t20 t01 "
    "t41 f61 f21 t02 f30 f62 t42 f31 f22 f70 t51 f72 f52 f71 t11 f53 f13 f32 f23 f03 f12 f43 f63 f73 "
    "f33 "
)
_PROG[1] = (
    "x01 x03 x31 x33 s713 s130 s613 s110 s133 x02 h110 x32 s623 s120 s020 s030 h710 h610 h010 h011 "
    "h611 h111 h711 s010 s033 s633 w32 h720 h620 h320 h020 / h120 w31 h021 h721 h310 h321 h621 h630 "
    "h730 h311 h121 h130 h030 w60 s603 w70 w10 s100 h031 h731 / h131 h631 w30 w00 s000 s733 s703 w50 "
    "s723 h300 h500 h700 / h600 h000 w33 w40 h001 h101 h401 h331 h100 h601 h330 h701 h301 h400 h501 "
    "w42 w52 w21 w22 o00 h421 h521 h221 p00 o70 o60 h420 h220 h520 p60 p70 o30 o10 h210 a30 e30 p10 "
    "w51 w41 w20 o11 o61 / o31 o71 p61 p11 o01 h200 h511 h411 h211 p01 p71 h510 h410 w43 a31 e31 w23 "
    "w53 o02 h230 h430 h530 p02 h531 o62 o50 p62 a50 o72 e50 h431 h201 o40 p72 a40 e40 h231 o52 o20 "
    "p52 a20 e20 a21 a22 a32 o63 o41 p63 a41 o53 e41 o43 o51 p43 a51 e51 p53 o73 o42 a42 p73 e42 a33 "
    "a23 a12 o23 o21 t21 o12 o33 e23 a13 t30 o22 o03 e22 t31 o13 o32 e33 t22 e32 a03 e12 t32 f10 e13 "
    "t12 e03 t23 t40 t03 t20 t41 t51 t13 f00 t50 e21 t33 t42 f63 f01 f70 f60 f61 f62 f73 f02 f72 f11 "
    "f71 f53 f52 f43 "
)
_PROG[3] = (
    "x00 s102 s101 x02 s001 x20 x22 s502 s402 s002 s122 x01 s501 s022 s401 s521 s421 h000 h400 x21 "
    "h401 h501 h500 h101 h410 h010 h510 h100 h001 w71 s012 w61 w31 w21 s112 s411 s511 h311 h310 h611 "
    "/ h711 h111 h011 h411 h210 h710 h110 h211 h511 h610 w22 w53 w13 w62 s531 h521 h620 h120 h520 "
    "s132 h121 h421 h420 h020 h021 h220 h221 h621 w23 w03 w43 w63 s431 s032 h131 h530 h230 h130 h030 "
    "h631 h031 h531 h431 h430 w20 w60 o50 o10 / o00 o40 p10 p50 h600 / h200 h630 h231 h201 h601 p40 "
    "p00 o60 / o20 w70 p20 w73 w32 p60 w72 w33 w30 o41 o01 h320 o51 o11 p01 p41 h331 h730 o61 o21 p51 "
    "h301 p11 o02 o42 h300 h700 p42 p02 h720 h701 a30 a70 a21 a61 h321 e61 e21 h330 h731 h721 o30 / "
    "o70 a71 e30 e70 a31 o71 o31 o22 o32 e71 e31 o62 o72 a22 a62 t71 e62 e22 o52 o12 a32 a72 e32 e72 "
    "o03 a52 a12 e12 e52 o23 o63 o13 a63 a23 e23 e63 o43 t70 a03 a43 o73 e03 e43 t31 o53 a53 e53 a13 "
    "o33 e13 a33 e33 a73 t30 e73 t63 t23 t22 t62 t33 t73 t32 t72 t12 t52 t13 t53 t43 t03 f11 f50 f00 "
    "f60 f41 f01 f51 f40 f20 t21 t61 f02 f10 f42 "
)


def _targets():
    tgt = [[None] * _NT for _ in range(4)]
    for u in range(_NT):
        name = _ROUTE[u % 16]
        if u >= 16:
            name = {"A": "B", "B": "A"}[name[0]] + name[1:]
        a, b, c, e = _PATHS[name[:2]]
        fwd = name[2] == "f"
        tgt[a][u] = (b, e if fwd else None)
        tgt[b][u] = (c, a)
        tgt[c][u] = (b, None if fwd else e)
        tgt[e][u] = (c, None)
    return tgt


def _chip_plan(d):
    src = 1 if d == 2 else d
    steps = [(t[0],) + tuple(int(ch) for ch in t[1:]) for t in _PROG[src].split()]
    xloads = _XLOADS[src]
    if d == 2:
        def mirror(s):
            if s[0] == "/":
                return s
            if s[0] == "x":
                return (s[0], (s[1] + 2) % 4) + s[2:]
            return (s[0], (s[1] + 4) % 8) + s[2:]
        steps = [mirror(s) for s in steps]
        xloads = tuple(((b + 2) % 4, k0, nk) for b, k0, nk in xloads)
    return steps, xloads, _W1ORDER[src]


def _fuse(steps, w1order):
    ops, w1_seen, w2_seen, cast, synced = [], 0, 0, set(), False
    i = 0
    while i < len(steps):
        s = steps[i]
        if s[0] == "/":
            i += 1
        elif s[0] in "ho":
            j = i
            while j < len(steps) and steps[j][0] == s[0] and steps[j][2:] == s[2:]:
                j += 1
            if s[0] == "h":
                need = 2 * w1order.index(s[2]) + s[3] + 1
                waits = range(w1_seen, need)
                w1_seen = max(w1_seen, need)
            else:
                waits = range(w2_seen, s[2] + 1)
                w2_seen = max(w2_seen, s[2] + 1)
            key = (s[0],) + s[2:]
            ops.append(dict(kind=s[0], arg=s[2:], groups=[t[1] for t in steps[i:j]], waits=list(waits),
                            cast=key not in cast, send=False,
                            small=not waits and j - i <= (4 if s[0] == "h" else 2)))
            cast.add(key)
            i = j
        else:
            sync = s[0] == "s" and not synced
            synced = synced or sync
            ops.append(dict(kind=s[0], arg=s[1:], sync=sync, early=False, send=s[0] in "pes" and not sync))
            i += 1
    for i, o in enumerate(ops):
        if not o["send"]:
            continue
        j = i - 1
        while ops[j]["send"] and ops[j]["early"]:
            j -= 1
        mm, before = ops[j], ops[j - 1]
        if mm["kind"] not in "ho" or not mm["small"]:
            continue
        if mm["kind"] == "o" and o["kind"] != "s" and mm["arg"][0] == o["arg"][1] and o["arg"][0] in mm["groups"]:
            continue
        if before["kind"] in "aw":
            n = len(mm["groups"])
            o["early"] = n == 1 if mm["kind"] == "o" else (n <= 2 and not mm["cast"])
        else:
            o["early"] = before["kind"] in "ho" or (before["send"] and before["early"])
    return ops


def _compiler_params():
    try:
        return pltpu.CompilerParams(collective_id=0, disable_semaphore_checks=True)
    except TypeError:
        return pltpu.CompilerParams(collective_id=0)


def pallas_dist_mlp2_tp_i_m512_h1024_out512_kernel(x, W1, W2):
    assert x.shape == (_M, _K) and W1.shape == (_K, _H) and W2.shape == (_H, _N)
    tgt = _targets()
    plans = [_chip_plan(d) for d in range(4)]

    def body(x_hbm, w1_hbm, w2_hbm, out_ref, x32, x16, w1_32, w1_16, w2_32, w2_16, acc, h16,
             sbuf, rbuf, load_sem, x_sem, recv_sem, send_sem):
        me = lax.axis_index("i")
        barrier = pltpu.get_barrier_semaphore()

        def load_w1(d, n):
            ix = (pl.ds(plans[d][2][n // 2] * _KC, _KC), pl.ds((n % 2) * _HC, _HC))
            return pltpu.make_async_copy(w1_hbm.at[ix], w1_32.at[ix], load_sem.at[n])

        def load_w2(q):
            return pltpu.make_async_copy(w2_hbm.at[:, pl.ds(q * _QC, _QC)], w2_32.at[q], load_sem.at[8 + q])

        def load_x(d, n):
            b, k0, nk = plans[d][1][n]
            ix = (pl.ds(b * _RB, _RB), pl.ds(k0 * _KC, nk * _KC))
            return pltpu.make_async_copy(x_hbm.at[ix], x32.at[ix], load_sem.at[12 + n])

        def prologue(d):
            load_x(d, 0).start()
            for p in _NBRS[d]:
                pl.semaphore_signal(barrier, inc=1, device_id=(_POS[p],), device_id_type=_MESH)
            for n in range(1, len(plans[d][1])):
                load_x(d, n).start()
            for n in range(8):
                load_w1(d, n).start()
            for q in range(4):
                load_w2(q).start()

        def program(d):
            steps, xloads, w1order = plans[d]
            path_end = set(4 * s[1] + s[2] for s in steps if s[0] == "p")
            h_count = {}
            x_ok, x_loaded, partial, arrived, summed, final = set(), set(), set(), set(), set(), set()
            sent = []

            def rdma(src, dst, sem, p):
                return pltpu.make_async_remote_copy(src, dst, send_sem.at[len(sent)], sem,
                                                    device_id=(_POS[p],), device_id_type=_MESH)

            def start(copy):
                copy.start()
                sent.append(copy)

            def x_copy(r, k, p):
                piece = x16.at[k, pl.ds(r * _RG, _RG), :]
                return rdma(piece, piece, x_sem.at[4 * r + k], p)

            def send(src, slot, p):
                assert sent and p in _NBRS[d]
                start(rdma(src, rbuf.at[slot], recv_sem.at[slot], p))

            def receive(slot):
                rdma(sbuf.at[slot], rbuf.at[slot], recv_sem.at[slot], _NBRS[d][0]).wait_recv()

            def tile(u):
                return (pl.ds((u // 4) * _RG, _RG), pl.ds((u % 4) * _QC, _QC))

            def rows(load, groups):
                runs = []
                for g in groups:
                    if runs and sum(runs[-1]) == g:
                        runs[-1][1] += 1
                    else:
                        runs.append([g, 1])
                parts = [load(pl.ds(g * _RG, n * _RG)) for g, n in runs]
                return parts[0] if len(parts) == 1 else jnp.concatenate(parts, axis=0)

            def add_partner(u, v):
                v = v + rbuf[u].astype(_F32)
                out_ref[tile(u)] = v
                sbuf[u] = v.astype(_BF16)
                summed.add(u)

            def store_result(o, res):
                for j, g in enumerate(o["groups"]):
                    v = res[j * _RG:(j + 1) * _RG]
                    if o["kind"] == "h":
                        half = o["arg"][1]
                        ix = (pl.ds(g * _RG, _RG), pl.ds(half * _HC, _HC))
                        n = h_count.get((g, half), 0)
                        if n == 0:
                            acc[ix] = v
                        elif n < 3:
                            acc[ix] += v
                        else:
                            h16[ix] = jnp.maximum(acc[ix] + v, 0.0).astype(_BF16)
                        h_count[(g, half)] = n + 1
                    else:
                        u = 4 * g + o["arg"][0]
                        if u in path_end:
                            sbuf[u] = v.astype(_BF16)
                        elif u in arrived:
                            add_partner(u, v)
                        else:
                            out_ref[tile(u)] = v
                        partial.add(u)

            def weights(o, w32, w16, ix):
                if not o["cast"]:
                    return w16[ix]
                w = w32[ix].astype(_BF16)
                w16[ix] = w
                return w

            pending, drained = None, 0
            ops = _fuse(steps, w1order)
            for i, o in enumerate(ops):
                kind, arg = o["kind"], o["arg"]
                if len(ops) - i in _DRAIN_AT:
                    upto = max(drained, len(sent) - _DRAIN_AT[len(ops) - i])
                    for copy in sent[drained:upto]:
                        copy.wait_send()
                    drained = upto
                if pending is not None and not (o["send"] and o["early"]):
                    store_result(*pending)
                    pending = None
                if kind == "h":
                    k, half = arg
                    assert all((g, k) in x_ok for g in o["groups"])
                    for n in o["waits"]:
                        load_w1(d, n).wait()
                    w = weights(o, w1_32, w1_16, (pl.ds(k * _KC, _KC), pl.ds(half * _HC, _HC)))
                    lhs = rows(lambda r: x16[k, r, :], o["groups"])
                    pending = (o, jnp.dot(lhs, w, preferred_element_type=_F32))
                elif kind == "o":
                    assert all(h_count[(g, half)] == 4 for g in o["groups"] for half in range(2))
                    for q in o["waits"]:
                        load_w2(q).wait()
                    w = weights(o, w2_32, w2_16, arg[0])
                    lhs = rows(lambda r: h16[r, :], o["groups"])
                    pending = (o, jnp.dot(lhs, w, preferred_element_type=_F32))
                elif kind == "x":
                    b, k = arg
                    n = [k0 <= k < k0 + nk and bb == b for bb, k0, nk in xloads].index(True)
                    if n not in x_loaded:
                        load_x(d, n).wait()
                        x_loaded.add(n)
                    blk = pl.ds(b * _RB, _RB)
                    x16[k, blk, :] = x32[blk, pl.ds(k * _KC, _KC)].astype(_BF16)
                    x_ok.update(((2 * b, k), (2 * b + 1, k)))
                elif kind == "s":
                    r, k, p = arg
                    if o["sync"]:
                        pl.semaphore_wait(barrier, 2)
                    assert (r, k) in x_ok and p in _NBRS[d] and (sent or o["sync"])
                    start(x_copy(r, k, p))
                elif kind == "w":
                    x_copy(arg[0], arg[1], _NBRS[d][0]).wait_recv()
                    x_ok.add(arg)
                else:
                    u = 4 * arg[0] + arg[1]
                    first, second = tgt[d][u]
                    if kind == "p":
                        assert u in partial
                        send(sbuf.at[u], u, first)
                    elif kind == "a":
                        receive(u)
                        arrived.add(u)
                        if u in partial:
                            add_partner(u, out_ref[tile(u)])
                    elif kind == "e":
                        assert u in summed
                        send(sbuf.at[u], _NT + u, first)
                    elif kind == "t":
                        assert u in summed
                        receive(_NT + u)
                        v = out_ref[tile(u)] + rbuf[_NT + u].astype(_F32)
                        if second is not None:
                            sbuf[_NT + u] = v.astype(_BF16)
                            send(sbuf.at[_NT + u], _NT + u, second)
                        out_ref[tile(u)] = v
                        final.add(u)
                    else:
                        assert kind == "f"
                        receive(_NT + u)
                        if second is not None:
                            send(rbuf.at[_NT + u], _NT + u, second)
                        out_ref[tile(u)] = rbuf[_NT + u].astype(_F32)
                        final.add(u)
            assert pending is None and len(final) == _NT and len(x_ok) == 32
            assert len(x_loaded) == len(xloads)
            for copy in sent[drained:]:
                copy.wait_send()

        for fn in (prologue, program):
            for d in (1, 2, 3, 0):
                pl.when(me == _POS[d])(functools.partial(fn, d))

    return pl.pallas_call(
        body,
        out_shape=jax.ShapeDtypeStruct((_M, _N), _F32),
        in_specs=[pl.BlockSpec(memory_space=pl.ANY)] * 3,
        out_specs=pl.BlockSpec(memory_space=pltpu.VMEM),
        scratch_shapes=[
            pltpu.VMEM((_M, _K), _F32),
            pltpu.VMEM((_K // _KC, _M, _KC), _BF16),
            pltpu.VMEM((_K, _H), _F32),
            pltpu.VMEM((_K, _H), _BF16),
            pltpu.VMEM((_N // _QC, _H, _QC), _F32),
            pltpu.VMEM((_N // _QC, _H, _QC), _BF16),
            pltpu.VMEM((_M, _H), _F32),
            pltpu.VMEM((_M, _H), _BF16),
            pltpu.VMEM((2 * _NT, _RG, _QC), _BF16),
            pltpu.VMEM((2 * _NT, _RG, _QC), _BF16),
            pltpu.SemaphoreType.DMA((16,)),
            pltpu.SemaphoreType.DMA((32,)),
            pltpu.SemaphoreType.DMA((2 * _NT,)),
            pltpu.SemaphoreType.DMA((72,)),
        ],
        compiler_params=_compiler_params(),
    )(x, W1, W2)
```
